```python
import numpy as np

kernel_name = "dist_sparse_attn_blocksparse_qseq_kvseq_b2_sq256_skv256_hq4_dh64"

def setup_inputs():
    x = np.random.randn(2, 1024, 512).astype(np.float32)
    Wq = np.random.randn(512, 256).astype(np.float32) * 0.02
    K_ext = np.random.randn(2, 1024, 4, 64).astype(np.float32)
    V_ext = np.random.randn(2, 1024, 4, 64).astype(np.float32)
    Wo = np.random.randn(256, 512).astype(np.float32) * 0.02
    return {"x": x, "Wq": Wq, "K_ext": K_ext, "V_ext": V_ext, "Wo": Wo}

def reference(x, Wq, K_ext, V_ext, Wo):
    B, Sq, Skv, Hq, Dh = 2, 1024, 1024, 4, 64
    Q = (x @ Wq).reshape(B, Sq, Hq, Dh)
    qb = (np.arange(Sq) // 64)[:, None]
    kb = (np.arange(Skv) // 64)[None, :]
    mask = (qb == kb) | (kb == 0) | ((qb + kb) % 3 == 0)
    scores = np.einsum('bihd,bjhd->bhij', Q, K_ext).astype(np.float32) * 0.125
    scores = np.where(mask[None, None, :, :], scores, -1e9)
    scores_max = scores.max(axis=-1, keepdims=True)
    w = np.exp(scores - scores_max)
    row_keep = mask.any(axis=1)
    w_sum = np.where(row_keep[None, None, :, None], w.sum(axis=-1, keepdims=True), 1.0)
    w = w / w_sum
    w = np.where(row_keep[None, None, :, None], w, 0.0)
    ctx = np.einsum('bhij,bjhd->bihd', w, V_ext).reshape(B, Sq, Hq * Dh)
    return ctx @ Wo
```

```python
import jax
import jax.numpy as jnp
from jax import lax
from jax.experimental import pallas as pl
from jax.experimental.pallas import tpu as pltpu

BF = jnp.bfloat16
F32 = jnp.float32
NEG = -1e30
NT = (((1,), (1,)), ((), ()))
MESH = pl.DeviceIdType.MESH
QSCALE = 0.125 * 1.4426950408889634

PRI = ((3, 1, 2), (0, 3, 2), (0, 3, 1), (0, 1, 2))
REGIONS = (
    (('L', 0), ('L', 1)),
    (('L', 2), ('A', 0), ('B', 0)),
    (('L', 3), ('A', 1)),
    (('A', 2), ('B', 2), ('B', 1)),
    (('A', 3), ('B', 3), ('O', 3)),
    (('O', 0), ('O', 1), ('O', 2)),
)
Q_ORDER = (
    ((2, 0), (1, 1), (2, 1), (2, 2), (1, 3), (3, 0), (1, 0), (3, 1), (2, 3), (1, 2), (3, 2), (3, 3)),
    ((3, 0), (3, 1), (0, 0), (0, 3), (0, 1), (2, 0), (3, 2), (2, 1), (0, 2), (2, 3), (3, 3), (2, 2)),
    ((0, 0), (0, 2), (1, 0), (3, 2), (0, 1), (0, 3), (1, 1), (3, 0), (1, 2), (3, 1), (1, 3), (3, 3)),
    ((0, 0), (0, 1), (1, 0), (0, 2), (1, 1), (0, 3), (1, 2), (2, 0), (2, 1), (2, 2), (2, 3), (1, 3)),
)
N_Q_FIRST = (6, 4, 4, 3)
N_Q_SECOND = (0, 4, 2, 5)
V_WAIT = ((1, 2, 3), (0, 2, 3), (3,), (0,))
KV_OPS = (
    ('Kd', 'Ks', 'Vs', 'Vd', 'KD', 'VD'),
    ('Ks', 'Kd', 'KD', 'Vs', 'Vd', 'VD'),
    ('KD', 'Kd', 'Ks', 'VD', 'Vs', 'Vd'),
    ('Kd', 'Ks', 'KD', 'Vd', 'VD', 'Vs'),
)


def _sel_lanes(a, b):
    a32 = pltpu.bitcast(a, jnp.uint32)
    b32 = pltpu.bitcast(b, jnp.uint32)
    lane = lax.broadcasted_iota(jnp.int32, a32.shape, 1)
    return pltpu.bitcast(jnp.where(lane < 64, a32, b32), BF)


def _roll64(a):
    return pltpu.bitcast(pltpu.roll(pltpu.bitcast(a, jnp.uint32), 64, 1), BF)


def _gather_classes(buf, c_ref):
    t = [buf[1, i] for i in range(8)]
    c_ref[0] = _sel_lanes(t[0], t[1])
    c_ref[1] = _sel_lanes(t[3], t[4])
    c_ref[2] = _sel_lanes(t[6], t[7])
    c_ref[3] = _sel_lanes(t[1], t[2])
    c_ref[4] = _sel_lanes(t[4], t[5])
    c_ref[5] = _sel_lanes(t[7], _roll64(t[0]))
    c_ref[6] = _sel_lanes(t[2], t[0])
    c_ref[7] = _sel_lanes(t[5], t[3])
    c_ref[8] = _sel_lanes(t[0], t[6])


def _mod3(v):
    v = jnp.where(v < 0, v + 3, v)
    return jnp.where(v >= 3, v - 3, v)


def _blk_info(s, slot):
    if slot < 3:
        i = _mod3(slot - _mod3(s))
        return slot, 2 * s + (i >> 1), i & 1
    cls = _mod3(s)
    return cls, 2 * s + 1, jnp.where(cls == 0, 2, 1)


def _scores(s, slot, qbuf, kbuf, kc):
    cls, tile, half = _blk_info(s, slot)
    q32 = pltpu.bitcast(qbuf[1, s * 4 + slot], jnp.uint32)
    lane32 = lax.broadcasted_iota(jnp.int32, (32, 128), 1)
    z = jnp.zeros_like(q32)
    q0 = pltpu.bitcast(jnp.where(lane32 < 64, q32, z), BF)
    q1 = pltpu.bitcast(jnp.where(lane32 < 64, z, q32), BF)
    qq = jnp.concatenate([q0, q1], axis=0)
    tiles = [jnp.dot(qq, kc[3 * cls + j], preferred_element_type=F32) for j in range(3)]
    if slot != 0:
        sd = jnp.dot(qq, kbuf[1, tile], preferred_element_type=F32)
        lane = lax.broadcasted_iota(jnp.int32, (128, 128), 1)
        tiles.append(jnp.where((lane >> 6) == half, sd, NEG))
    return tiles


def _softmax(tiles):
    mx = tiles[0]
    for t in tiles[1:]:
        mx = jnp.maximum(mx, t)
    m = jnp.max(mx, axis=1, keepdims=True)
    ps = [jnp.exp2(t - m) for t in tiles]
    sm = ps[0]
    for p in ps[1:]:
        sm = sm + p
    l = jnp.sum(sm, axis=1, keepdims=True)
    lo = lax.broadcasted_iota(jnp.int32, (64, 128), 1) < 64
    lsel = jnp.where(lo, l[0:64], l[64:128])
    return [p.astype(BF) for p in ps], 1.0 / lsel


def _context(s, slot, probs, vbuf, vc):
    ps, rinv = probs
    cls, tile, _ = _blk_info(s, slot)
    vt = [vc[3 * cls + j] for j in range(3)] + ([vbuf[1, tile]] if slot != 0 else [])
    o = None
    for p, v in zip(ps, vt):
        d = lax.dot_general(p, v, NT, preferred_element_type=F32)
        o = d if o is None else o + d
    lo = lax.broadcasted_iota(jnp.int32, (64, 128), 1) < 64
    return (jnp.where(lo, o[0:64], o[64:128]) * rinv).astype(BF)


def _kernel(x_hbm, wq_hbm, kt_hbm, vt_hbm, wo_hbm, out_ref,
            kf, vf, xf, wqf, wof, wob, kbuf, vbuf, qbuf, cbuf, kc, vc,
            ld_sem, ks_sem, kr_sem, vs_sem, vr_sem, qs_sem, qr_sem, cs_sem, cr_sem, ent_sem):
    me = lax.axis_index("i")

    def dev(k):
        return lax.rem(me + k, 4)

    def pick(vals):
        r = vals[3]
        for p in (2, 1, 0):
            r = jnp.where(me == p, vals[p], r)
        return r

    src_of = {"O": me}
    for n, role in enumerate("LAB"):
        src_of[role] = pick([PRI[p][n] for p in range(4)])

    kld = {k: pltpu.make_async_copy(kt_hbm.at[dev(k)], kf.at[dev(k)], ld_sem.at[k]) for k in range(4)}
    vld = {k: pltpu.make_async_copy(vt_hbm.at[dev(k)], vf.at[dev(k)], ld_sem.at[4 + k]) for k in range(4)}
    wq_ld = pltpu.make_async_copy(wq_hbm, wqf, ld_sem.at[8])
    x_ld = [pltpu.make_async_copy(x_hbm.at[b], xf.at[b], ld_sem.at[9 + b]) for b in range(2)]
    wo_ld = pltpu.make_async_copy(wo_hbm, wof, ld_sem.at[11])

    def kv_send(buf, j, ssem, rsem):
        return pltpu.make_async_remote_copy(
            buf.at[0, pl.ds(j * 2, 2)], buf.at[1, pl.ds(me * 2, 2)], ssem.at[j], rsem.at[me],
            device_id=(j,), device_id_type=MESH)

    def kv_recv(buf, src, ssem, rsem):
        return pltpu.make_async_remote_copy(
            buf.at[0, pl.ds(src * 2, 2)], buf.at[1, pl.ds(src * 2, 2)], ssem.at[src], rsem.at[src],
            device_id=(src,), device_id_type=MESH)

    def blk_send(buf, j, slot, ssem, rsem):
        return pltpu.make_async_remote_copy(
            buf.at[0, j * 4 + slot], buf.at[1, me * 4 + slot],
            ssem.at[j * 4 + slot], rsem.at[me * 4 + slot], device_id=(j,), device_id_type=MESH)

    def blk_recv(buf, src, slot, ssem, rsem):
        return pltpu.make_async_remote_copy(
            buf.at[0, src * 4 + slot], buf.at[1, src * 4 + slot],
            ssem.at[src * 4 + slot], rsem.at[src * 4 + slot], device_id=(src,), device_id_type=MESH)

    def kv_convert(f, buf, k):
        j = dev(k)
        sel = 1 if k == 0 else 0
        v = f[j]
        buf[sel, j * 2] = v[:, 0:128].astype(BF)
        buf[sel, j * 2 + 1] = v[:, 128:256].astype(BF)

    bs = pltpu.get_barrier_semaphore()

    def peer(p, c):
        return {"s": p ^ 1, "d": p ^ 3, "D": p ^ 2}[c]

    def prologue(p, signal_to, early, n_signals):
        kseq = [peer(p, op[1]) for op in KV_OPS[p] if op[0] == "K"]
        vseq = [peer(p, op[1]) for op in KV_OPS[p] if op[0] == "V"]
        rel = lambda d: (d - p) % 4
        for d in signal_to:
            pl.semaphore_signal(bs, inc=1, device_id=(d,), device_id_type=MESH)
        for d in kseq + [p]:
            kld[rel(d)].start()
        for d in vseq + [p]:
            vld[rel(d)].start()
        wq_ld.start()
        for c in x_ld:
            c.start()
        wo_ld.start()

        done_k, done_v = set(), set()

        def conv_k(d):
            if d not in done_k:
                done_k.add(d)
                kld[rel(d)].wait()
                kv_convert(kf, kbuf, rel(d))

        def conv_v(d):
            if d not in done_v:
                done_v.add(d)
                vld[rel(d)].wait()
                kv_convert(vf, vbuf, rel(d))

        late = [d for d in kseq if d not in early]
        if late:
            for d in kseq:
                if d in early:
                    conv_k(d)
        pl.semaphore_wait(bs, n_signals)
        if not late:
            for d in (p ^ 2, p ^ 1, p ^ 3):
                pl.semaphore_signal(ent_sem, inc=1, device_id=(d,), device_id_type=MESH)
        entered = not late
        for op in KV_OPS[p]:
            d = peer(p, op[-1])
            if d not in early and not entered:
                for d2 in late:
                    conv_k(d2)
                pl.semaphore_wait(ent_sem, 1)
                entered = True
            if op[0] == "K":
                conv_k(d)
                kv_send(kbuf, d, ks_sem, kr_sem).start()
            elif op[0] == "V":
                conv_v(d)
                kv_send(vbuf, d, vs_sem, vr_sem).start()
            elif op[1] == "K":
                kv_send(kbuf, d, ks_sem, kr_sem).wait_send()
            else:
                kv_send(vbuf, d, vs_sem, vr_sem).wait_send()

    for p, args in enumerate((((1, 3, 2), (1, 3), 2), ((0, 2), (0,), 1), ((), (0, 1, 3), 3), ((0, 2), (0,), 1))):
        @pl.when(me == p)
        def _(p=p, args=args):
            prologue(p, *args)

    kld[0].wait()
    kv_convert(kf, kbuf, 0)
    vld[0].wait()
    kv_convert(vf, vbuf, 0)

    wq_ld.wait()
    for c in x_ld:
        c.wait()
    wq = wqf[...].astype(BF)
    for b in range(2):
        qf = jnp.dot(xf[b].astype(BF), wq, preferred_element_type=F32) * QSCALE
        for g in range(2):
            j = 2 * b + g
            sel = (me == j).astype(jnp.int32)
            for i in range(4):
                slot = _mod3(i + _mod3(me)) if i < 3 else 3
                qbuf[sel, j * 4 + slot] = qf[64 * i:64 * i + 64, 128 * g:128 * g + 128].astype(BF)

    def waited_in_prologue(p, kind):
        return [peer(p, op[2]) for op in KV_OPS[p] if op[:2] == "W" + kind]

    def issue_q(lo, hi, wait_v=False):
        for p in range(4):
            msgs = Q_ORDER[p][lo[p]:hi[p]]
            waits = [d for d in V_WAIT[p] if d not in waited_in_prologue(p, "V")] if wait_v else []
            if msgs or waits:
                @pl.when(me == p)
                def _(msgs=msgs, waits=waits):
                    for d in waits:
                        kv_send(vbuf, d, vs_sem, vr_sem).wait_send()
                    for d, slot in msgs:
                        blk_send(qbuf, d, slot, qs_sem, qr_sem).start()

    n_two = tuple(a + b for a, b in zip(N_Q_FIRST, N_Q_SECOND))
    issue_q((0,) * 4, N_Q_FIRST)

    wo_ld.wait()
    for kt in range(2):
        for nt in range(4):
            wob[kt * 4 + nt] = wof[128 * kt:128 * kt + 128, 128 * nt:128 * nt + 128].astype(BF)

    for k in (1, 3, 2):
        kv_recv(kbuf, dev(k), ks_sem, kr_sem).wait_recv()
    _gather_classes(kbuf, kc)
    own_scores = [_scores(me, slot, qbuf, kbuf, kc) for slot in range(4)]
    probs = {("O", slot): _softmax(own_scores[slot]) for slot in range(4)}

    issue_q(N_Q_FIRST, n_two)
    issue_q(n_two, (12,) * 4, wait_v=True)

    for k in (1, 3, 2):
        kv_recv(vbuf, dev(k), vs_sem, vr_sem).wait_recv()

    for n, region in enumerate(REGIONS):
        for role, slot in region:
            if role != "O":
                blk_recv(qbuf, src_of[role], slot, qs_sem, qr_sem).wait_recv()
        if n == 0:
            _gather_classes(vbuf, vc)
        todo = [b for b in region if b not in probs]
        scores = {b: _scores(src_of[b[0]], b[1], qbuf, kbuf, kc) for b in todo}
        for b in todo:
            probs[b] = _softmax(scores.pop(b))
        for role, slot in region:
            s = src_of[role]
            cbuf[1 if role == "O" else 0, s * 4 + slot] = _context(s, slot, probs.pop((role, slot)), vbuf, vc)
        for role, slot in region:
            if role != "O":
                blk_send(cbuf, src_of[role], slot, cs_sem, cr_sem).start()

    for k in (1, 2, 3):
        for slot in range(4):
            blk_send(qbuf, dev(k), slot, qs_sem, qr_sem).wait_send()
    for p in range(4):
        rest_k = [d for d in range(4) if d != p and d not in waited_in_prologue(p, "K")]
        rest_v = [d for d in range(4) if d != p and d not in V_WAIT[p] and d not in waited_in_prologue(p, "V")]

        @pl.when(me == p)
        def _(rest_k=rest_k, rest_v=rest_v):
            for d in rest_k:
                kv_send(kbuf, d, ks_sem, kr_sem).wait_send()
            for d in rest_v:
                kv_send(vbuf, d, vs_sem, vr_sem).wait_send()

    for slot in range(4):
        if slot == 3:
            for k in (1, 2, 3):
                for sl in range(4):
                    blk_send(cbuf, dev(k), sl, cs_sem, cr_sem).wait_send()
        for k in (1, 3, 2):
            blk_recv(cbuf, dev(k), slot, cs_sem, cr_sem).wait_recv()
        i = _mod3(slot - _mod3(me)) if slot < 3 else 3
        rows = pl.ds(pl.multiple_of(64 * i, 64), 64)
        a0 = jnp.concatenate([cbuf[1, 0 + slot], cbuf[1, 8 + slot]], axis=0)
        a1 = jnp.concatenate([cbuf[1, 4 + slot], cbuf[1, 12 + slot]], axis=0)
        for nt in range(4):
            o = (jnp.dot(a0, wob[nt], preferred_element_type=F32)
                 + jnp.dot(a1, wob[4 + nt], preferred_element_type=F32))
            out_ref[0, rows, 128 * nt:128 * nt + 128] = o[0:64]
            out_ref[1, rows, 128 * nt:128 * nt + 128] = o[64:128]


def pallas_dist_sparse_attn_blocksparse_qseq_kvseq_b2_sq256_skv256_hq4_dh64_kernel(
    x: jax.Array,
    Wq: jax.Array,
    K_ext: jax.Array,
    V_ext: jax.Array,
    Wo: jax.Array,
):
    kt = jnp.transpose(K_ext, (0, 2, 3, 1)).reshape(4, 128, 256)
    vt = jnp.transpose(V_ext, (0, 2, 3, 1)).reshape(4, 128, 256)
    any_spec = pl.BlockSpec(memory_space=pl.ANY)
    dma = pltpu.SemaphoreType.DMA
    return pl.pallas_call(
        _kernel,
        out_shape=pltpu.MemorySpace.VMEM((2, 256, 512), F32),
        in_specs=[any_spec] * 5,
        out_specs=pl.BlockSpec(memory_space=pltpu.VMEM),
        scratch_shapes=[
            pltpu.VMEM((4, 128, 256), F32), pltpu.VMEM((4, 128, 256), F32),
            pltpu.VMEM((2, 256, 512), F32),
            pltpu.VMEM((512, 256), F32), pltpu.VMEM((256, 512), F32),
            pltpu.VMEM((8, 128, 128), BF),
            pltpu.VMEM((2, 8, 128, 128), BF), pltpu.VMEM((2, 8, 128, 128), BF),
            pltpu.VMEM((2, 16, 64, 128), BF), pltpu.VMEM((2, 16, 64, 128), BF),
            pltpu.VMEM((9, 128, 128), BF), pltpu.VMEM((9, 128, 128), BF),
            dma((12,)), dma((4,)), dma((4,)), dma((4,)), dma((4,)),
            dma((16,)), dma((16,)), dma((16,)), dma((16,)),
            pltpu.SemaphoreType.REGULAR,
        ],
        compiler_params=pltpu.CompilerParams(
            collective_id=0, vmem_limit_bytes=64 * 1024 * 1024,
            disable_semaphore_checks=True),
    )(x, Wq, kt, vt, Wo)
```
